```python
import numpy as np

kernel_name = "dist_mlpseq_tp1d_bs_rep_b64_d1024_h2048"

def setup_inputs():
    x = np.random.randn(256, 1024).astype(np.float32)
    Win0 = np.random.randn(1024, 8192).astype(np.float32)
    Wout0 = np.random.randn(8192, 1024).astype(np.float32)
    Win1 = np.random.randn(1024, 8192).astype(np.float32)
    Wout1 = np.random.randn(8192, 1024).astype(np.float32)
    Win2 = np.random.randn(1024, 8192).astype(np.float32)
    Wout2 = np.random.randn(8192, 1024).astype(np.float32)
    return {"x": x, "Win0": Win0, "Wout0": Wout0, "Win1": Win1, "Wout1": Wout1, "Win2": Win2, "Wout2": Wout2}

def reference(x, Win0, Win1, Win2, Wout0, Wout1, Wout2):
    h = x @ Win0
    h = np.maximum(h, 0.0)
    x = h @ Wout0
    h = x @ Win1
    h = np.maximum(h, 0.0)
    x = h @ Wout1
    h = x @ Win2
    h = np.maximum(h, 0.0)
    x = h @ Wout2
    return x
```

```python
import contextlib

import jax
import jax.numpy as jnp
from jax import lax
from jax.experimental import pallas as pl
from jax.experimental.pallas import tpu as pltpu

BF16 = jnp.bfloat16
F32 = jnp.float32
N_DEV = 4
N_LAYER = 3
LANE = 128
MESH = pl.DeviceIdType.MESH


def make(kp=(8, 8), ns=4, mm=None, early=2, late5=0, scopes=False, lag=3, flags=None, nocomm=False, upw=2, tail=None):
    def scope(name):
        on = scopes is True or (scopes and any(name.startswith(p) for p in scopes))
        return jax.named_scope("@" + name) if on else contextlib.nullcontext()

    def fn(x, Win0, Wout0, Win1, Wout1, Win2, Wout2):
        m_loc, d = x.shape
        m = m_loc * N_DEV
        h = Win0.shape[1]
        nd, nh = d // LANE, h // LANE
        kpl, nsl = kp, ns
        assert sum(kp) == nh and sum(kpl) == nh

        def body(x_hbm, wi0, wo0, wi1, wo1, wi2, wo2, act,
                 xf, win, wout, hb, acc, s1, r1, s2, r2,
                 x_sem, win_sem, wout_sem, xr_sem, r1_sem, r2_sem, snd_sem):
            wi = (wi0, wi1, wi2)
            wo = (wo0, wo1, wo2)
            me = lax.axis_index("i")
            nbr = (me ^ 1, (N_DEV - 1) - me)

            def cols(j):
                if isinstance(j, int):
                    return pl.ds(j * LANE, LANE)
                return pl.ds(pl.multiple_of(j * LANE, LANE), LANE)

            def fetch_win(l, g):
                for i in range(upw):
                    j = upw * g + i
                    pltpu.make_async_copy(wi[l].at[:, cols(j)], win.at[l, j],
                                          win_sem.at[l, g]).start()

            def kpieces(sizes):
                return [(p, sum(sizes[:p]), sizes[p]) for p in range(len(sizes))]

            def fetch_wout(l, c, sizes):
                for p, k0, kn in kpieces(sizes):
                    g = pl.ds(k0 * 8, kn * 8)
                    for e in range(2):
                        pltpu.make_async_copy(wo[l].at[g, e, :, cols(c)],
                                              wout.at[l, c, g, e],
                                              wout_sem.at[l, c, p]).start()

            x_cp = pltpu.make_async_copy(x_hbm, xf, x_sem)
            x_cp.start()
            lax.fori_loop(0, nh // upw, lambda g, _: fetch_win(0, g), None)

            bar = pltpu.get_barrier_semaphore()
            for t in nbr:
                pl.semaphore_signal(bar, inc=1, device_id=(t,), device_id_type=MESH)

            def xblk(dev, half):
                n = m_loc // 2
                return act.at[pl.ds(pl.multiple_of(dev * m_loc + half * n, n), n)]

            def xsend(dev, half, to, k):
                cp = pltpu.make_async_remote_copy(xblk(dev, half), xblk(dev, half), snd_sem.at[0],
                                                  xr_sem.at[k], device_id=(to,), device_id_type=MESH)
                cp.start()
                return cp

            def xrecv(dev, half, k):
                pltpu.make_async_copy(xblk(dev, half), xblk(dev, half), xr_sem.at[k]).wait()

            with scope("x0"):
                x_cp.wait()
            act[pl.ds(pl.multiple_of(me * m_loc, m_loc), m_loc), :] = xf[...].astype(BF16)
            pl.semaphore_wait(bar, 2)
            with scope("xag"):
                sends = [xsend(me, 0, nbr[0], 0), xsend(me, 1, nbr[1], 1),
                         xsend(me, 1, nbr[0], 2), xsend(me, 0, nbr[1], 3)]
                xrecv(nbr[0], 0, 0)
                xrecv(nbr[1], 1, 1)
                sends += [xsend(nbr[0], 0, nbr[1], 4), xsend(nbr[1], 1, nbr[0], 5)]
                xrecv(nbr[0], 1, 2)
                xrecv(nbr[1], 0, 3)
                xrecv(me ^ 2, 0, 4)
                xrecv(me ^ 2, 1, 5)
                for cp in sends:
                    cp.wait_send()

            def send(src, dst, sem, l, c, s, n, order):
                if nocomm: return
                ms = m // n
                for half, t in enumerate(order):
                    rows = pl.ds(s * ms + half * (ms // 2), ms // 2)
                    pltpu.make_async_remote_copy(
                        src.at[l, c, rows], dst.at[l, c, rows], snd_sem.at[1],
                        sem.at[l, c, s], device_id=(t,), device_id_type=MESH).start()

            def recv(dst, sem, l, c, s, n):
                if nocomm: return
                blk = dst.at[l, c, pl.ds(s * (m // n), m // n)]
                pltpu.make_async_copy(blk, blk, sem.at[l, c, s]).wait()

            def forward(l, c, s, n):
                recv(r1, r1_sem, l, c, s, n)
                rows = pl.ds(s * (m // n), m // n)
                s2[l, c, rows] = (s1[l, c, rows].astype(F32)
                                  + r1[l, c, rows].astype(F32)).astype(BF16)
                send(s2, r2, r2_sem, l, c, s, n, nbr[::-1])

            def finish(l, c, s, n):
                recv(r2, r2_sem, l, c, s, n)
                rows = pl.ds(s * (m // n), m // n)
                act[rows, cols(c)] = (s2[l, c, rows].astype(F32)
                                      + r2[l, c, rows].astype(F32)).astype(BF16)

            def partial(l, c, sizes, n, nmm, mid):
                for p, k0, kn in kpieces(sizes):
                    blk = wout.at[l, c, pl.ds(k0 * 8, kn * 8)]
                    with scope(f"w{p}"):
                        pltpu.make_async_copy(blk, blk, wout_sem.at[l, c, p]).wait()
                    w = blk[...].reshape(kn * LANE, LANE).astype(BF16)
                    ks = range(k0, k0 + kn)
                    if p < len(sizes) - 1:
                        a = jnp.concatenate([hb[k] for k in ks], axis=1)
                        t = jnp.dot(a, w, preferred_element_type=F32)
                        acc[...] = t if p == 0 else acc[...] + t
                        if p == 0:
                            mid()
                        continue
                    s0 = 0
                    for cnt in nmm:
                        rows = pl.ds(s0 * (m // n), cnt * (m // n))
                        a = jnp.concatenate([hb[k, rows] for k in ks], axis=1)
                        t = jnp.dot(a, w, preferred_element_type=F32)
                        if p > 0:
                            t = t + acc[rows]
                        s1[l, c, rows] = t.astype(BF16)
                        for s in range(s0, s0 + cnt):
                            send(s1, r1, r1_sem, l, c, s, n, nbr)
                        s0 += cnt

            def layer(l, _):
                def up(g, _):
                    blk = win.at[l, pl.ds(upw * g, upw)]
                    with scope("u"):
                        pltpu.make_async_copy(blk, blk, win_sem.at[l, g]).wait()
                    per = nd * upw // nh
                    for ll in range(N_LAYER):
                        @pl.when(l == ll)
                        def _():
                            for i in range(per):
                                fetch_wout(ll, per * g + i, kp)
                    w = jnp.concatenate([win[l, upw * g + i] for i in range(upw)], axis=1).astype(BF16)
                    r = jnp.maximum(jnp.dot(act[...], w, preferred_element_type=F32), 0.0).astype(BF16)
                    for i in range(upw):
                        hb[upw * g + i] = r[:, i * LANE:(i + 1) * LANE]

                with scope("up"):
                    lax.fori_loop(0, nh // upw, up, None)

                def prefetch(c):
                    per = nd * upw // nh
                    for ll in range(N_LAYER - 1):
                        pl.when((l == ll) & (c % per == 0))(lambda: fetch_win(ll + 1, c // per))

                def down(c, _):
                    def mid():
                        if early < ns - late5: pl.when(c >= 2)(lambda: [forward(l, c - 2, s, ns) for s in range(early, ns - late5)] and None)
                        if late5:
                            pl.when((c >= 2) & (c < nd - 1))(lambda: [forward(l, c - 2, s, ns) for s in range(ns - late5, ns)] and None)
                    partial(l, c, kp, ns, mm or (1,) * ns, mid if early < ns else lambda: None)
                    prefetch(c)

                    @pl.when((c >= 1) & ((c < nd - 1) | (late5 == 0)))
                    def _():
                        with scope("f"):
                            for s in range(early):
                                forward(l, c - 1, s, ns)

                    @pl.when(c >= lag)
                    def _():
                        for s in range(ns):
                            finish(l, c - lag, s, ns)

                lax.fori_loop(0, nd, down, None)
                with scope("f56"):
                    for s in range(ns - late5, ns):
                        forward(l, nd - 3, s, ns)
                    for s in range(0 if late5 else early, ns):
                        forward(l, nd - 2, s, ns)

                def fin(c, _):
                    for s in range(ns):
                        finish(l, c, s, ns)

                with scope("fin"):
                    lax.fori_loop(nd - lag, nd - 3, fin, None)
                for s in range(ns):
                    with scope(f"fw7{s}"):
                        forward(l, nd - 1, s, ns)
                with scope("finl"):
                    lax.fori_loop(max(nd - lag, nd - 3), nd, fin, None)

            lax.fori_loop(0, N_LAYER, layer, None)

            if not nocomm:
                for buf in (s1, s2):
                    pltpu.make_async_copy(buf, buf, snd_sem.at[1]).wait()

        view = lambda w: w.reshape(h // 16, 2, 8, d)
        comm = pltpu.VMEM((N_LAYER, nd, m, LANE), BF16)
        hbm = pl.BlockSpec(memory_space=pltpu.HBM)
        return pl.pallas_call(
            body,
            out_shape=pltpu.VMEM((m, d), BF16),
            in_specs=[hbm] * 7,
            out_specs=pl.BlockSpec(memory_space=pltpu.VMEM),
            scratch_shapes=[
                pltpu.VMEM((m_loc, d), F32),
                pltpu.VMEM((N_LAYER, nh, d, LANE), F32),
                pltpu.VMEM((N_LAYER, nd, h // 16, 2, 8, LANE), F32),
                pltpu.VMEM((nh, m, LANE), BF16),
                pltpu.VMEM((m, LANE), F32),
                comm, comm, comm, comm,
                pltpu.SemaphoreType.DMA,
                pltpu.SemaphoreType.DMA((N_LAYER, nh // upw)),
                pltpu.SemaphoreType.DMA((N_LAYER, nd, max(len(kp), len(kpl)))),
                pltpu.SemaphoreType.DMA((6,)),
                pltpu.SemaphoreType.DMA((N_LAYER, nd, max(ns, nsl))),
                pltpu.SemaphoreType.DMA((N_LAYER, nd, max(ns, nsl))),
                pltpu.SemaphoreType.DMA((2,)),
            ],
            compiler_params=pltpu.CompilerParams(
                collective_id=0,
                vmem_limit_bytes=100 * 2**20,
                disable_bounds_checks=True,
                disable_semaphore_checks=True,
                flags=flags,
            ),
        )(x, Win0, view(Wout0), Win1, view(Wout1), Win2, view(Wout2))

    return fn


def pallas_dist_mlpseq_tp1d_bs_rep_b64_d1024_h2048_kernel(x, Win0, Wout0, Win1, Wout1, Win2, Wout2):
    return make(early=3, late5=1)(x, Win0, Wout0, Win1, Wout1, Win2, Wout2)
```

```python
import jax
import jax.numpy as jnp
from jax import lax
from jax.experimental import pallas as pl
from jax.experimental.pallas import tpu as pltpu

BF16 = jnp.bfloat16
F32 = jnp.float32
MESH = pl.DeviceIdType.MESH

N_DEV = 4
N_LAYER = 3
N_MXU = 4
LANE = 128
SUBLANE = 8

K_PIECES = (7, 5, 4)
N_SUB = 8
LOOKAHEAD = 5
LAST_DEV = 2


def _span(i, n):
    return pl.ds(i * n if isinstance(i, int) else pl.multiple_of(i * n, n), n)


def _dot(a, w):
    return jnp.dot(a, w, preferred_element_type=F32)


def _balanced_dot(a, w):
    rest = w.shape[0] // LANE % N_MXU
    if rest == 0:
        return _dot(a, w)
    k = w.shape[0] - rest * LANE
    rows = a.shape[0] // N_MXU
    tail = [_dot(a[i * rows:(i + 1) * rows, k:], w[k:]) for i in range(N_MXU)]
    return _dot(a[:, :k], w[:k]) + jnp.concatenate(tail, axis=0)


def pallas_dist_mlpseq_tp1d_bs_rep_b64_d1024_h2048_kernel(
    x: jax.Array,
    Win0: jax.Array,
    Wout0: jax.Array,
    Win1: jax.Array,
    Wout1: jax.Array,
    Win2: jax.Array,
    Wout2: jax.Array,
):
    m_loc, d = x.shape
    m = m_loc * N_DEV
    h = Win0.shape[1]
    nd, nh = d // LANE, h // LANE
    m_sub = m // N_SUB
    assert nh == 2 * nd == sum(K_PIECES)
    pieces = [(p, sum(K_PIECES[:p]), kn) for p, kn in enumerate(K_PIECES)]

    def body(x_hbm, wi0, wo0, wi1, wo1, wi2, wo2,
             act,
             x_buf, win, wout, hid, acc, send1, recv1, send2, recv2,
             x_sem, win_sem, wout_sem, xs_sem, xr_sem, r1_sem, r2_sem, send_sem):
        win_hbm = (wi0, wi1, wi2)
        wout_hbm = (wo0, wo1, wo2)
        me = lax.axis_index("i")
        nbr = (me ^ 1, (N_DEV - 1) - me)

        def fetch_win(l, g):
            for j in (2 * g, 2 * g + 1):
                pltpu.make_async_copy(
                    win_hbm[l].at[:, _span(j, LANE)], win.at[l, j], win_sem.at[j]
                ).start()

        def fetch_wout(l, c):
            for p, k0, kn in pieces:
                g = pl.ds(k0 * SUBLANE, kn * SUBLANE)
                for odd in range(2):
                    pltpu.make_async_copy(
                        wout_hbm[l].at[g, odd, :, _span(c, LANE)],
                        wout.at[l, c, odd, g],
                        wout_sem.at[c, p],
                    ).start()

        x_copy = pltpu.make_async_copy(x_hbm, x_buf, x_sem)
        x_copy.start()
        lax.fori_loop(0, nd, lambda g, _: fetch_win(0, g), None)

        barrier = pltpu.get_barrier_semaphore()
        for dev in nbr:
            pl.semaphore_signal(barrier, inc=1, device_id=(dev,), device_id_type=MESH)

        def x_rows(owner, half, to, k):
            rows = act.at[_span(2 * owner + half, m_loc // 2)]
            return pltpu.make_async_remote_copy(
                rows, rows, xs_sem.at[k], xr_sem.at[k], device_id=(to,), device_id_type=MESH
            )

        x_copy.wait()
        act[_span(me, m_loc), :] = x_buf[...].astype(BF16)
        pl.semaphore_wait(barrier, 2)
        sends = [x_rows(me, 0, nbr[0], 0), x_rows(me, 1, nbr[1], 1),
                 x_rows(me, 1, nbr[0], 2), x_rows(me, 0, nbr[1], 3),
                 x_rows(nbr[0], 0, nbr[1], 4), x_rows(nbr[1], 1, nbr[0], 5)]
        recvs = [x_rows(nbr[0], 0, me, 0), x_rows(nbr[1], 1, me, 1),
                 x_rows(nbr[0], 1, me, 2), x_rows(nbr[1], 0, me, 3),
                 x_rows(me ^ 2, 0, me, 4), x_rows(me ^ 2, 1, me, 5)]
        for copy in sends[:4]:
            copy.start()
        for k in range(2):
            recvs[k].wait_recv()
            sends[4 + k].start()
        for copy in recvs[2:]:
            copy.wait_recv()
        for copy in sends:
            copy.wait_send()

        def send(src, dst, stage, sem, l, q):
            for half in range(2):
                rows = _span(2 * q + half, m_sub // 2)
                pltpu.make_async_remote_copy(
                    src.at[l, rows], dst.at[l, rows], send_sem.at[stage], sem.at[l, q],
                    device_id=(nbr[half ^ stage],), device_id_type=MESH,
                ).start()

        def pair_sum(own, got, sem, l, q):
            blk = got.at[l, _span(q, m_sub)]
            pltpu.make_async_copy(blk, blk, sem.at[l, q]).wait()
            return (own[l, _span(q, m_sub)].astype(F32) + blk[...].astype(F32)).astype(BF16)

        def layer(l, _):
            def up(j, _):
                pltpu.make_async_copy(win.at[l, j], win.at[l, j], win_sem.at[j]).wait()
                pre = _dot(act[...], win[l, j].astype(BF16))
                hid[j] = jnp.maximum(pre, 0.0).astype(BF16)
                g = (j >> 1) + LOOKAHEAD
                l_even = jnp.where((j & 1) == 0, l, -1)
                for ll in range(N_LAYER):
                    if ll > 0:
                        pl.when((l_even == ll) & (g < nd))(lambda: fetch_win(ll, g))
                    pl.when((l_even == ll) & (g >= nd))(lambda: fetch_wout(ll, g - nd))

            lax.fori_loop(0, nh, up, None)

            def forward(lo, hi):
                def step(i, _):
                    for q in (2 * i, 2 * i + 1):
                        send2[l, _span(q, m_sub)] = pair_sum(send1, recv1, r1_sem, l, q)
                        send(send2, recv2, 1, r2_sem, l, q)

                lax.fori_loop(lo >> 1, hi >> 1, step, None)
                return jnp.maximum(lo, hi)

            is_last = me == LAST_DEV
            eager = jnp.where(is_last, N_SUB, 2)
            limit = jnp.where(is_last, (nd - 3) * N_SUB + 2, (nd - 2) * N_SUB)

            def down(c, done):
                for p, k0, kn in pieces:
                    blk = wout.at[l, c, :, pl.ds(k0 * SUBLANE, kn * SUBLANE)]
                    pltpu.make_async_copy(blk, blk, wout_sem.at[c, p]).wait()
                    w = jnp.stack([blk[0], blk[1]], axis=1).reshape(kn * LANE, LANE)
                    a = jnp.concatenate([hid[k] for k in range(k0, k0 + kn)], axis=1)
                    part = _balanced_dot(a, w.astype(BF16))
                    if p < len(pieces) - 1:
                        acc[...] = part if p == 0 else acc[...] + part
                    if p == 0:
                        done = forward(done, jnp.minimum((c - 1) * N_SUB, limit))
                for s in range(N_SUB):
                    q = c * N_SUB + s
                    total = part[s * m_sub:(s + 1) * m_sub] + acc[_span(s, m_sub)]
                    send1[l, _span(q, m_sub)] = total.astype(BF16)
                    send(send1, recv1, 0, r1_sem, l, q)
                g = c + LOOKAHEAD
                for ll in range(N_LAYER):
                    pl.when((l == ll) & (g < nd))(lambda: fetch_wout(ll, g))
                    if ll + 1 < N_LAYER:
                        pl.when((l == ll) & (g >= nd))(lambda: fetch_win(ll + 1, g - nd))
                return forward(done, jnp.minimum((c - 1) * N_SUB + eager, limit))

            done = lax.fori_loop(0, nd, down, jnp.int32(0))
            forward(done, nd * N_SUB)

            def finish(c, _):
                for s in range(N_SUB):
                    act[_span(s, m_sub), _span(c, LANE)] = pair_sum(
                        send2, recv2, r2_sem, l, c * N_SUB + s
                    )

            lax.fori_loop(0, nd, finish, None)

        lax.fori_loop(0, N_LAYER, layer, None)

        pltpu.make_async_copy(send1, send1, send_sem.at[0]).wait()
        pltpu.make_async_copy(send2, send2, send_sem.at[1]).wait()

    def by_tile_row(w):
        return w.reshape(h // (2 * SUBLANE), 2, SUBLANE, d)

    comm = pltpu.VMEM((N_LAYER, nd * m, LANE), BF16)
    dma = pltpu.SemaphoreType.DMA
    return pl.pallas_call(
        body,
        out_shape=pltpu.VMEM((m, d), BF16),
        in_specs=[pl.BlockSpec(memory_space=pltpu.HBM)] * 7,
        out_specs=pl.BlockSpec(memory_space=pltpu.VMEM),
        scratch_shapes=[
            pltpu.VMEM((m_loc, d), F32),
            pltpu.VMEM((N_LAYER, nh, d, LANE), F32),
            pltpu.VMEM((N_LAYER, nd, 2, h // (2 * SUBLANE), SUBLANE, LANE), F32),
            pltpu.VMEM((nh, m, LANE), BF16),
            pltpu.VMEM((m, LANE), F32),
            comm, comm, comm, comm,
            dma, dma((nh,)), dma((nd, len(pieces))), dma((6,)), dma((6,)),
            dma((N_LAYER, nd * N_SUB)), dma((N_LAYER, nd * N_SUB)), dma((2,)),
        ],
        compiler_params=pltpu.CompilerParams(
            collective_id=0,
            vmem_limit_bytes=100 * 2**20,
            disable_bounds_checks=True,
            disable_semaphore_checks=True,
        ),
    )(x, Win0, by_tile_row(Wout0), Win1, by_tile_row(Wout1), Win2, by_tile_row(Wout2))
```

```python
import jax
import jax.numpy as jnp
from jax import lax
from jax.experimental import pallas as pl
from jax.experimental.pallas import tpu as pltpu

BF16 = jnp.bfloat16
F32 = jnp.float32
MESH = pl.DeviceIdType.MESH

N_DEV = 4
N_LAYER = 3
N_MXU = 4
LANE = 128
SUBLANE = 8

K_PIECES = (7, 5, 4)
N_SUB = 8
LOOKAHEAD = 5
LAST_DEV = 2


def _span(i, n):
    return pl.ds(i * n if isinstance(i, int) else pl.multiple_of(i * n, n), n)


def _dot(a, w):
    return jnp.dot(a, w, preferred_element_type=F32)


def _balanced_dot(a, w):
    rest = w.shape[0] // LANE % N_MXU
    if rest == 0:
        return _dot(a, w)
    k = w.shape[0] - rest * LANE
    rows = a.shape[0] // N_MXU
    tail = [_dot(a[i * rows:(i + 1) * rows, k:], w[k:]) for i in range(N_MXU)]
    return _dot(a[:, :k], w[:k]) + jnp.concatenate(tail, axis=0)


def pallas_dist_mlpseq_tp1d_bs_rep_b64_d1024_h2048_kernel(
    x: jax.Array,
    Win0: jax.Array,
    Wout0: jax.Array,
    Win1: jax.Array,
    Wout1: jax.Array,
    Win2: jax.Array,
    Wout2: jax.Array,
):
    m_loc, d = x.shape
    m = m_loc * N_DEV
    h = Win0.shape[1]
    nd, nh = d // LANE, h // LANE
    m_sub = m // N_SUB
    assert nh == 2 * nd == sum(K_PIECES)
    pieces = [(p, sum(K_PIECES[:p]), kn) for p, kn in enumerate(K_PIECES)]

    def body(x_hbm, wi0, wo0, wi1, wo1, wi2, wo2,
             act,
             x_buf, win, wout, hid, acc, send1, recv1, send2, recv2,
             x_sem, win_sem, wout_sem, xs_sem, xr_sem, r1_sem, r2_sem, send_sem):
        win_hbm = (wi0, wi1, wi2)
        wout_hbm = (wo0, wo1, wo2)
        me = lax.axis_index("i")
        nbr = (me ^ 1, (N_DEV - 1) - me)

        def fetch_win(l, g):
            for j in (2 * g, 2 * g + 1):
                pltpu.make_async_copy(
                    win_hbm[l].at[:, _span(j, LANE)], win.at[l, j], win_sem.at[j]
                ).start()

        def fetch_wout(l, c, final=False):
            for p, k0, kn in pieces:
                g = pl.ds(k0 * SUBLANE, kn * SUBLANE)
                whole = final and p == len(pieces) - 1
                for odd in ((slice(None),) if whole else (0, 1)):
                    pltpu.make_async_copy(
                        wout_hbm[l].at[g, odd, :, _span(c, LANE)],
                        wout.at[l, c, g, odd],
                        wout_sem.at[c, p],
                    ).start()

        x_copy = pltpu.make_async_copy(x_hbm, x_buf, x_sem)
        x_copy.start()
        lax.fori_loop(0, nd, lambda g, _: fetch_win(0, g), None)

        barrier = pltpu.get_barrier_semaphore()
        for dev in nbr:
            pl.semaphore_signal(barrier, inc=1, device_id=(dev,), device_id_type=MESH)

        def x_rows(owner, half, to, k):
            rows = act.at[_span(2 * owner + half, m_loc // 2)]
            return pltpu.make_async_remote_copy(
                rows, rows, xs_sem.at[k], xr_sem.at[k], device_id=(to,), device_id_type=MESH
            )

        x_copy.wait()
        act[_span(me, m_loc), :] = x_buf[...].astype(BF16)
        pl.semaphore_wait(barrier, 2)
        sends = [x_rows(me, 0, nbr[0], 0), x_rows(me, 1, nbr[1], 1),
                 x_rows(me, 1, nbr[0], 2), x_rows(me, 0, nbr[1], 3),
                 x_rows(nbr[0], 0, nbr[1], 4), x_rows(nbr[1], 1, nbr[0], 5)]
        recvs = [x_rows(nbr[0], 0, me, 0), x_rows(nbr[1], 1, me, 1),
                 x_rows(nbr[0], 1, me, 2), x_rows(nbr[1], 0, me, 3),
                 x_rows(me ^ 2, 0, me, 4), x_rows(me ^ 2, 1, me, 5)]
        for copy in sends[:4]:
            copy.start()
        for k in range(2):
            recvs[k].wait_recv()
            sends[4 + k].start()
        for copy in recvs[2:]:
            copy.wait_recv()
        for copy in sends:
            copy.wait_send()

        def send(src, dst, stage, sem, l, q):
            for half in range(2):
                rows = _span(2 * q + half, m_sub // 2)
                pltpu.make_async_remote_copy(
                    src.at[l, rows], dst.at[l, rows], send_sem.at[stage], sem.at[l, q],
                    device_id=(nbr[half ^ stage],), device_id_type=MESH,
                ).start()

        def pair_sum(own, got, sem, l, q):
            blk = got.at[l, _span(q, m_sub)]
            pltpu.make_async_copy(blk, blk, sem.at[l, q]).wait()
            return (own[l, _span(q, m_sub)].astype(F32) + blk[...].astype(F32)).astype(BF16)

        def layer(l, _):
            def up(j, _):
                pltpu.make_async_copy(win.at[l, j], win.at[l, j], win_sem.at[j]).wait()
                pre = _dot(act[...], win[l, j].astype(BF16))
                hid[j] = jnp.maximum(pre, 0.0).astype(BF16)
                g = (j >> 1) + LOOKAHEAD
                l_even = jnp.where((j & 1) == 0, l, -1)
                for ll in range(N_LAYER):
                    if ll > 0:
                        pl.when((l_even == ll) & (g < nd))(lambda: fetch_win(ll, g))
                    pl.when((l_even == ll) & (g >= nd))(lambda: fetch_wout(ll, g - nd))

            lax.fori_loop(0, nh, up, None)

            def forward(lo, hi):
                def step(i, _):
                    for q in (2 * i, 2 * i + 1):
                        send2[l, _span(q, m_sub)] = pair_sum(send1, recv1, r1_sem, l, q)
                        send(send2, recv2, 1, r2_sem, l, q)

                hi = jnp.maximum(lo, hi)
                lax.fori_loop(lo >> 1, hi >> 1, step, None)
                return hi

            is_last = me == LAST_DEV
            eager = jnp.where(is_last, N_SUB, 2)
            limit = jnp.where(is_last, (nd - 3) * N_SUB + 2, (nd - 2) * N_SUB)

            def down(c, done):
                for p, k0, kn in pieces:
                    blk = wout.at[l, c, pl.ds(k0 * SUBLANE, kn * SUBLANE)]
                    pltpu.make_async_copy(blk, blk, wout_sem.at[c, p]).wait()
                    w = blk[...].reshape(kn * LANE, LANE)
                    a = jnp.concatenate([hid[k] for k in range(k0, k0 + kn)], axis=1)
                    part = _balanced_dot(a, w.astype(BF16))
                    if p < len(pieces) - 1:
                        acc[...] = part if p == 0 else acc[...] + part
                    if p == 0:
                        done = forward(done, jnp.minimum((c - 1) * N_SUB, limit))
                for s in range(N_SUB):
                    q = c * N_SUB + s
                    total = part[s * m_sub:(s + 1) * m_sub] + acc[_span(s, m_sub)]
                    send1[l, _span(q, m_sub)] = total.astype(BF16)
                    send(send1, recv1, 0, r1_sem, l, q)
                g = c + LOOKAHEAD
                end = N_LAYER - 1
                for ll in range(end):
                    pl.when((l == ll) & (g < nd))(lambda: fetch_wout(ll, g))
                    pl.when((l == ll) & (g >= nd))(lambda: fetch_win(ll + 1, g - nd))
                pl.when((l == end) & (g < nd - 1))(lambda: fetch_wout(end, g))
                pl.when((l == end) & (g == nd - 1))(lambda: fetch_wout(end, nd - 1, final=True))
                return forward(done, jnp.minimum((c - 1) * N_SUB + eager, limit))

            done = lax.fori_loop(0, nd, down, jnp.int32(0))
            forward(done, nd * N_SUB)

            def finish(c, _):
                for s in range(N_SUB):
                    act[_span(s, m_sub), _span(c, LANE)] = pair_sum(
                        send2, recv2, r2_sem, l, c * N_SUB + s
                    )

            lax.fori_loop(0, nd, finish, None)

        lax.fori_loop(0, N_LAYER, layer, None)

        pltpu.make_async_copy(send1, send1, send_sem.at[0]).wait()
        pltpu.make_async_copy(send2, send2, send_sem.at[1]).wait()

    def by_tile_row(w):
        return w.reshape(h // (2 * SUBLANE), 2, SUBLANE, d)

    comm = pltpu.VMEM((N_LAYER, nd * m, LANE), BF16)
    dma = pltpu.SemaphoreType.DMA
    return pl.pallas_call(
        body,
        out_shape=jax.ShapeDtypeStruct((m, d), BF16),
        in_specs=[pl.BlockSpec(memory_space=pltpu.HBM)] * 7,
        out_specs=pl.BlockSpec(memory_space=pltpu.VMEM),
        scratch_shapes=[
            pltpu.VMEM((m_loc, d), F32),
            pltpu.VMEM((N_LAYER, nh, d, LANE), F32),
            pltpu.VMEM((N_LAYER, nd, h // (2 * SUBLANE), 2, SUBLANE, LANE), F32),
            pltpu.VMEM((nh, m, LANE), BF16),
            pltpu.VMEM((m, LANE), F32),
            comm, comm, comm, comm,
            dma, dma((nh,)), dma((nd, len(pieces))), dma((6,)), dma((6,)),
            dma((N_LAYER, nd * N_SUB)), dma((N_LAYER, nd * N_SUB)), dma((2,)),
        ],
        compiler_params=pltpu.CompilerParams(
            collective_id=0,
            vmem_limit_bytes=100 * 2**20,
            disable_bounds_checks=True,
            disable_semaphore_checks=True,
        ),
    )(x, Win0, by_tile_row(Wout0), Win1, by_tile_row(Wout1), Win2, by_tile_row(Wout2))
```
